```python
import numpy as np

kernel_name = "dist_sort_i_m128_n64"

def setup_inputs():
    return {"x": np.random.randn(512, 64).astype(np.float32)}

def reference(x: np.ndarray) -> np.ndarray:
    return np.sort(x, axis=0)
```

```python
import jax
import jax.numpy as jnp
from jax import lax
from jax.experimental import pallas as pl
from jax.experimental.pallas import tpu as pltpu

MESH = pl.DeviceIdType.MESH
F32 = jnp.float32
BF16 = jnp.bfloat16
U32 = jnp.uint32

_SORT16 = [
    [(0, 13), (1, 12), (2, 15), (3, 14), (4, 8), (5, 6), (7, 11), (9, 10)],
    [(0, 5), (1, 7), (2, 9), (3, 4), (6, 13), (8, 14), (10, 15), (11, 12)],
    [(0, 1), (2, 3), (4, 5), (6, 8), (7, 9), (10, 11), (12, 13), (14, 15)],
    [(0, 2), (1, 3), (4, 10), (5, 11), (6, 7), (8, 9), (12, 14), (13, 15)],
    [(1, 2), (3, 12), (4, 6), (5, 7), (8, 10), (9, 11), (13, 14)],
    [(1, 4), (2, 6), (5, 8), (7, 10), (9, 13), (11, 14)],
    [(2, 4), (3, 6), (9, 12), (11, 13)],
    [(3, 5), (6, 8), (7, 9), (10, 12)],
    [(3, 4), (5, 6), (7, 8), (9, 10), (11, 12)],
    [(6, 7), (8, 9)],
]
_ARRIVAL = [(0, 13, 5, 6), (1, 12, 7, 11), (2, 15, 9, 10), (3, 14, 4, 8)]

_SLOT = {
    0: {1: 0, 3: 1, 2: 2},
    1: {0: 0, 2: 1, 3: 2},
    3: {0: 0, 2: 1, 1: 2},
    2: {1: 0, 3: 1, 0: 2},
}


def _up(x, d):
    return pltpu.roll(x, (8 - d) % 8, 0)


class _Net:
    def __init__(self, sub):
        self.sub = sub
        self.masks = {}

    def mask(self, bits):
        if bits not in self.masks:
            x = self.sub & bits
            x = x ^ (x >> 2)
            x = x ^ (x >> 1)
            self.masks[bits] = (x & 1) == 0
        return self.masks[bits]

    def up(self, a, d):
        return _up(a[0], d), tuple(a[1][(s + d) % 8] for s in range(8))

    def sel(self, bits, a, b):
        even = [bin(s & bits).count("1") % 2 == 0 for s in range(8)]
        return (jnp.where(self.mask(bits), a[0], b[0]),
                tuple(a[1][s] if even[s] else b[1][s] for s in range(8)))

    def xor(self, a, d):
        if d == 4:
            return self.up(a, 4)
        return self.sel(d, self.up(a, d), self.up(a, 8 - d))

    @staticmethod
    def lo(a, b, mu):
        assert all(p ^ q == mu for p, q in zip(a[1], b[1])), (a[1], b[1], mu)
        return jnp.minimum(a[0], b[0]), tuple(min(p, q) for p, q in zip(a[1], b[1]))

    @staticmethod
    def hi(a, b, mu):
        assert all(p ^ q == mu for p, q in zip(a[1], b[1])), (a[1], b[1], mu)
        return jnp.maximum(a[0], b[0]), tuple(max(p, q) for p, q in zip(a[1], b[1]))

    @staticmethod
    def pairs(v, mu, d=0, first=None):
        out, used = [], set()
        order = sorted(range(len(v)), key=lambda i: (first is not None and bool(v[i][1][0] & first)))
        for i in order:
            if i in used:
                continue
            want = tuple(v[i][1][s ^ d] ^ mu for s in range(8))
            j = next(j for j in range(len(v)) if v[j][1] == want)
            assert j != i and j not in used
            used.update((i, j))
            out.append((v[i], v[j]))
        return out

    def align(self, v, mu, d, first):
        return [(a, self.xor(b, d) if d else b) for a, b in self.pairs(v, mu, d, first)]

    def stage(self, v, mu, d=0, first=None):
        out = []
        for a, b in self.align(v, mu, d, first):
            out += [self.lo(a, b, mu), self.hi(a, b, mu)]
        return out

    def swap(self, v, d, nu, bits):
        out = []
        for a, b in self.pairs(v, nu, first=nu):
            if d == 4:
                out.append((self.sel(bits, a, b), self.up(self.sel(bits, b, a), 4)))
            elif bits == d:
                out.append((self.sel(d, a, self.up(b, 8 - d)), self.sel(d, self.up(a, d), b)))
            else:
                out.append((self.sel(bits, a, b), self.xor(self.sel(bits, b, a), d)))
        return out

    def swap_stage(self, v, mu, d, nu, bits):
        out = []
        for a, b in self.swap(v, d, nu, bits):
            out += [self.lo(a, b, mu), self.hi(a, b, mu)]
        return out


def _ce(v, i, j, desc=False):
    lo = jnp.minimum(v[i], v[j])
    hi = jnp.maximum(v[i], v[j])
    v[i], v[j] = (hi, lo) if desc else (lo, hi)


def _vstage(v, d, desc=False):
    for i in range(len(v)):
        if not i & d:
            _ce(v, i, i | d, desc)


def _sstage(x, p_lo, p_hi, low, desc=False):
    if desc:
        return jnp.where(low, jnp.maximum(x, p_lo), jnp.minimum(x, p_hi))
    return jnp.where(low, jnp.minimum(x, p_lo), jnp.maximum(x, p_hi))


def pallas_dist_sort_i_m128_n64_kernel(x: jax.Array):
    xt = x.T

    def body(x_hbm, obuf, xin, sbuf, rbuf, lsem, ssem, rsem, rdy):
        me = lax.axis_index("i")
        cin = pltpu.make_async_copy(x_hbm, xin, lsem)
        cin.start()

        bar = pltpu.get_barrier_semaphore()

        def sig(sem, dst):
            pl.semaphore_signal(sem, inc=1, device_id=(dst,), device_id_type=MESH)

        @pl.when(me == 0)
        def _():
            sig(bar, 2); sig(bar, 1); sig(bar, 3)

        @pl.when(me == 2)
        def _():
            sig(bar, 0)
            pl.semaphore_wait(bar, 3)
            sig(rdy, 1); sig(rdy, 3)

        @pl.when(me % 2 == 1)
        def _():
            sig(bar, 2)
            pl.semaphore_wait(bar, 1)
            sig(rdy, 0)

        sub = lax.broadcasted_iota(jnp.int32, (8, 128), 0)
        lane = lax.broadcasted_iota(jnp.int32, (8, 128), 1)
        net = _Net(sub)
        s2lo, s1lo, s0lo = net.mask(4), net.mask(2), net.mask(1)
        hlo = lane < 64
        sgn = (1 - 2 * (me % 2)).astype(F32)
        nt = (((1,), (1,)), ((), ()))

        def eye_rows(q, val):
            ri = lax.broadcasted_iota(jnp.int32, (32, 128), 0) + 32 * q
            ci = lax.broadcasted_iota(jnp.int32, (32, 128), 1)
            return jnp.where(ri == ci, val, 0.0).astype(BF16)

        def transpose(w, val):
            return [lax.dot_general(eye_rows(q, val), w, nt, preferred_element_type=F32) for q in range(4)]

        def rcopy(src, dst, half=None):
            slot = _SLOT[dst][src]
            if half is None:
                s, d, k = sbuf, rbuf.at[slot], slot
            else:
                s, d, k = sbuf.at[pl.ds(16 * half, 16)], rbuf.at[slot, pl.ds(16 * half, 16)], slot + half
            return pltpu.make_async_remote_copy(
                src_ref=s, dst_ref=d, send_sem=ssem.at[k], recv_sem=rsem.at[k],
                device_id=(dst,), device_id_type=MESH)

        cin.wait()
        xb = xin[...].astype(BF16)
        ts = transpose(jnp.concatenate([xb, xb], axis=0), sgn)
        v = [None] * 16
        for p in range(4):
            for q in range(4):
                v[_ARRIVAL[p][q]] = ts[q][8 * p:8 * p + 8]
        for layer in _SORT16:
            for i, j in layer:
                _ce(v, i, j)
        v = [(v[i], tuple(i | (s >> 2) << 4 | ((s >> 1) & 1) << 5 | (s & 1) << 6 for s in range(8)))
             for i in range(16)]
        v = net.stage(v, 31, 4, first=1)
        for mu in (8, 4, 2):
            v = net.stage(v, mu)
        v = net.swap_stage(v, 1, 4, 2, 6)
        v = net.stage(v, 63, 2, first=1)
        for mu in (16, 8, 4):
            v = net.stage(v, mu)
        v = net.swap_stage(v, 2, 4, 4, 5)
        v = net.swap_stage(v, 1, 2, 2, 3)
        top = net.align(v, 127, 1, 1)

        def finish(h, half):
            for mu in (32, 16, 8):
                h = net.stage(h, mu)
            h = net.swap_stage(h, 4, 4, 8, 4)
            h = net.swap_stage(h, 2, 2, 4, 2)
            y = {}
            for a, b in net.swap(h, 1, 16, 1):
                lo, hi = net.lo(a, b, 1), net.hi(a, b, 1)
                base = lo[1][0]
                assert lo[1] == tuple(base | (s >> 2) << 3 | ((s >> 1) & 1) << 2 | (s & 1) << 4 for s in range(8))
                y[base & 63] = pltpu.bitcast(jnp.where(hlo, lo[0], hi[0]), U32)
            for e5 in range(2):
                sbuf[pl.ds(16 * half + 8 * e5, 8), :] = (y[32 * e5] >> 16) | y[32 * e5 + 2]

        finish([net.lo(a, b, 127) for a, b in top], 0)

        @pl.when(me == 2)
        def _():
            rcopy(2, 0, 0).start()

        finish([net.hi(a, b, 127) for a, b in top], 1)

        @pl.when(me == 2)
        def _():
            rcopy(2, 0, 1).start(); rcopy(2, 3).start(); rcopy(2, 1).start()

        @pl.when(me == 0)
        def _():
            pl.semaphore_wait(rdy, 2)
            rcopy(0, 1).start(); rcopy(0, 3).start()
            pl.semaphore_wait(bar, 1)
            rcopy(0, 2, 0).start(); rcopy(0, 2, 1).start()

        @pl.when(me == 1)
        def _():
            rcopy(1, 0).start()
            pl.semaphore_wait(rdy, 1)
            rcopy(1, 3, 0).start(); rcopy(1, 3, 1).start(); rcopy(1, 2).start()

        @pl.when(me == 3)
        def _():
            rcopy(3, 0).start()
            pl.semaphore_wait(rdy, 1)
            rcopy(3, 1, 0).start(); rcopy(3, 1, 1).start(); rcopy(3, 2).start()

        def unpack(ref, xor, halves=(0, 1)):
            out = []
            for e6 in halves:
                r = [None] * 4
                for e4 in range(2):
                    w = ref[pl.ds(16 * e6 + e4, 8, stride=2), :]
                    if xor is not None:
                        w = w ^ xor
                    f = pltpu.bitcast(w, BF16).astype(F32)
                    r[e4], r[2 + e4] = f[:8], f[8:]
                out += r
            return out

        def sub3(v, desc=False):
            out = []
            for a in v:
                r = _up(a, 4)
                a = _sstage(a, r, r, s2lo, desc)
                a = _sstage(a, _up(a, 2), _up(a, 6), s1lo, desc)
                a = _sstage(a, _up(a, 1), _up(a, 7), s0lo, desc)
                out.append(a)
            return out

        def merge7(v, desc=False):
            v = list(v)
            for d in (4, 2, 1):
                _vstage(v, d, desc)
            out = []
            for a in sub3(v, desc):
                r = pltpu.roll(a, 64, 1)
                out.append(_sstage(a, r, r, hlo, desc))
            return out

        def emit(v):
            v = list(v)
            for d in (2, 1):
                _vstage(v, d)
            z = []
            for p in sub3(v):
                w = pltpu.bitcast(p, U32)
                z.append(w | (w >> 16))
            zb = pltpu.bitcast(jnp.concatenate(z, axis=0), BF16)
            tt = transpose(zb, 1.0)
            ev = (lax.broadcasted_iota(jnp.int32, (32, 128), 1) & 1) == 0
            for q in range(2):
                obuf[pl.ds(32 * q, 32), :] = jnp.where(
                    ev, jnp.minimum(tt[q], tt[q + 2]), jnp.maximum(tt[q], tt[q + 2]))

        neg = jnp.uint32(0x80008000)
        own = unpack(sbuf, None)
        rcopy(1, 0).wait_recv()
        a = unpack(rbuf.at[0], neg)
        m0 = merge7([jnp.minimum(p, q) for p, q in zip(own, a)])
        m1 = merge7([jnp.maximum(p, q) for p, q in zip(own, a)])
        rcopy(3, 0).wait_recv()
        b = unpack(rbuf.at[1], neg)
        edge = jnp.logical_or(me == 0, me == 3)
        pp = [jnp.where(edge, jnp.minimum(p, q), jnp.maximum(p, q)) for p, q in zip(m0, b)]
        qq = [jnp.where(edge, -jnp.inf, p) for p in m1]
        u = merge7([jnp.maximum(p, q) for p, q in zip(pp, qq)], desc=True)
        l = merge7([jnp.minimum(p, q) for p, q in zip(pp, qq)], desc=True)
        u = [p * sgn for p in u]
        l = [p * sgn for p in l]
        lo = [jnp.minimum(p, q) for p, q in zip(u, l)]
        hi = [jnp.maximum(p, q) for p, q in zip(u, l)]
        dxor = (me % 2).astype(U32) * neg
        thr = jnp.where(sub == 7, _up(hi[4], 1), -jnp.inf)

        @pl.when(jnp.logical_or(me == 0, me == 1))
        def _():
            rcopy(1, 0).wait_send(); rcopy(1, 0).wait_send()

        @pl.when(jnp.logical_or(me == 2, me == 3))
        def _():
            rcopy(3, 0).wait_send(); rcopy(3, 0).wait_send()

        rcopy(2, 0, 0).wait_send(); rcopy(2, 0, 1).wait_send()

        rcopy(2, 0, 0).wait_recv()

        def fast():
            d = unpack(rbuf.at[2], None, halves=(0,))
            bad = jnp.max(jnp.where(d[3] < thr, 1.0, 0.0))
            f = [jnp.minimum(d[i], hi[4 + i]) for i in range(4)]
            f += [jnp.maximum(jnp.minimum(d[i], hi[i]), hi[4 + i]) for i in range(4)]
            emit(f)
            return (bad > 0.0).astype(jnp.int32)

        redo = lax.cond(me == 0, fast, lambda: jnp.int32(1))
        rcopy(2, 0, 1).wait_recv()

        @pl.when(redo != 0)
        def _():
            d = unpack(rbuf.at[2], dxor)
            f = [jnp.minimum(h, jnp.maximum(p, q)) for p, q, h in zip(d, lo, hi)]
            _vstage(f, 4)
            emit(f)

    out = pl.pallas_call(
        body,
        out_shape=jax.ShapeDtypeStruct((64, 128), F32),
        in_specs=[pl.BlockSpec(memory_space=pl.ANY)],
        out_specs=pl.BlockSpec(memory_space=pltpu.VMEM),
        scratch_shapes=[
            pltpu.VMEM((64, 128), F32),
            pltpu.VMEM((32, 128), U32),
            pltpu.VMEM((3, 32, 128), U32),
            pltpu.SemaphoreType.DMA,
            pltpu.SemaphoreType.DMA((4,)),
            pltpu.SemaphoreType.DMA((4,)),
            pltpu.SemaphoreType.REGULAR,
        ],
        compiler_params=pltpu.CompilerParams(collective_id=0, disable_semaphore_checks=True),
    )(xt)
    return out.T
```

```python
import jax
import jax.numpy as jnp
from jax import lax
from jax.experimental import pallas as pl
from jax.experimental.pallas import tpu as pltpu

MESH = pl.DeviceIdType.MESH
F32 = jnp.float32
BF16 = jnp.bfloat16
U32 = jnp.uint32

_SLOT = {
    0: {1: 0, 3: 1, 2: 2},
    1: {0: 0, 2: 1, 3: 2},
    3: {0: 0, 2: 1, 1: 2},
    2: {1: 0, 3: 1, 0: 2},
}
_HEAD_ROWS = 13


def _odd_even_merge(lo, n, r):
    m = 2 * r
    if m < n:
        yield from _odd_even_merge(lo, n, m)
        yield from _odd_even_merge(lo + r, n, m)
        for i in range(lo + r, lo + n - r, m):
            yield (i, i + r)
    else:
        yield (lo, lo + r)


_MERGE_8_8 = sorted(_odd_even_merge(0, 16, 1), key=lambda p: p[0] - p[1])


def _insertion_sort(xs):
    out = [xs[0]]
    for x in xs[1:]:
        mins = [jnp.minimum(p, x) for p in out] + [x]
        out = [mins[0]] + [jnp.maximum(p, q) for p, q in zip(out, mins[1:])]
    return out


def _perm(x, idx):
    return jnp.take_along_axis(x, idx, axis=0, mode="promise_in_bounds")


class _Net:
    def __init__(self, sub):
        self.low = {d: (sub & d) == 0 for d in (4, 2, 1)}
        self.idx = {d: sub ^ d for d in (1, 2, 6, 7)}

    def xor_val(self, x, d):
        return pltpu.roll(x, 4, 0) if d == 4 else _perm(x, self.idx[d])

    def xor(self, a, d):
        return self.xor_val(a[0], d), tuple(a[1][s ^ d] for s in range(8))

    def sel(self, d, a, b):
        return (jnp.where(self.low[d], a[0], b[0]),
                tuple(b[1][s] if s & d else a[1][s] for s in range(8)))

    @staticmethod
    def lo(a, b, mu):
        assert all(p ^ q == mu for p, q in zip(a[1], b[1]))
        return jnp.minimum(a[0], b[0]), tuple(min(p, q) for p, q in zip(a[1], b[1]))

    @staticmethod
    def hi(a, b, mu):
        assert all(p ^ q == mu for p, q in zip(a[1], b[1]))
        return jnp.maximum(a[0], b[0]), tuple(max(p, q) for p, q in zip(a[1], b[1]))

    @staticmethod
    def pairs(v, mu, d=0, first=0):
        out, used = [], set()
        for i in sorted(range(len(v)), key=lambda i: bool(v[i][1][0] & first)):
            if i in used:
                continue
            want = tuple(v[i][1][s ^ d] ^ mu for s in range(8))
            j = next(j for j in range(len(v)) if v[j][1] == want)
            assert j != i and j not in used
            used.update((i, j))
            out.append((v[i], v[j]))
        return out

    def align(self, v, mu, d, first):
        return [(a, self.xor(b, d) if d else b) for a, b in self.pairs(v, mu, d, first)]

    def both(self, pairs, mu):
        out = []
        for a, b in pairs:
            out += [self.lo(a, b, mu), self.hi(a, b, mu)]
        return out

    def stage(self, v, mu, d=0, first=0):
        return self.both(self.align(v, mu, d, first), mu)

    def swap(self, v, d, nu):
        return [(self.sel(d, a, b), self.xor(self.sel(d, b, a), d))
                for a, b in self.pairs(v, nu, first=nu)]

    def swap_stage(self, v, mu, d, nu):
        return self.both(self.swap(v, d, nu), mu)


def _ce(v, i, j, desc=False):
    lo = jnp.minimum(v[i], v[j])
    hi = jnp.maximum(v[i], v[j])
    v[i], v[j] = (hi, lo) if desc else (lo, hi)


def _vstage(v, d, desc=False):
    for i in range(len(v)):
        if not i & d:
            _ce(v, i, i | d, desc)


def _pick(low, x, p, desc=False):
    if desc:
        return jnp.where(low, jnp.maximum(x, p), jnp.minimum(x, p))
    return jnp.where(low, jnp.minimum(x, p), jnp.maximum(x, p))


def _rotate_regs(v, masks, sign=1):
    n = len(v)
    for b, m in enumerate(masks):
        v = [jnp.where(m, v[(k + sign * (1 << b)) % n], v[k]) for k in range(n)]
    return v


def _skew(x, base):
    return pltpu.roll(x, base, 1, stride=8, stride_axis=0)


def pallas_dist_sort_i_m128_n64_kernel(x: jax.Array):
    def body(x_hbm, obuf, xin, sbuf, rbuf, hbuf, tbuf, lsem, ssem, rsem, rdy):
        me = lax.axis_index("i")
        cin = pltpu.make_async_copy(x_hbm, xin, lsem)
        cin.start()

        bar = pltpu.get_barrier_semaphore()

        def sig(sem, dst):
            pl.semaphore_signal(sem, inc=1, device_id=(dst,), device_id_type=MESH)

        @pl.when(me == 0)
        def _():
            hbuf[pl.ds(8, 8), :] = jnp.full((8, 128), 0x7F807F80, U32)
            sig(bar, 2)
            sig(bar, 1)
            sig(bar, 3)

        @pl.when(me == 2)
        def _():
            sig(bar, 0)
            pl.semaphore_wait(bar, 3)
            sig(rdy, 1)
            sig(rdy, 3)

        @pl.when(me % 2 == 1)
        def _():
            sig(bar, 2)
            pl.semaphore_wait(bar, 1)
            sig(rdy, 0)
            cin.wait()
            xin[...] = -xin[...]

        sub = lax.broadcasted_iota(jnp.int32, (8, 128), 0)
        lane = lax.broadcasted_iota(jnp.int32, (8, 128), 1)
        net = _Net(sub)
        hlo = lane < 64
        lbit = [(lane & (1 << b)) != 0 for b in range(3)]
        idx_in = [(((lane + k) >> 3) + sub) & 7 for k in range(8)]

        def rcopy(src, dst):
            slot = _SLOT[dst][src]
            return pltpu.make_async_remote_copy(
                src_ref=sbuf, dst_ref=rbuf.at[slot], send_sem=ssem.at[dst], recv_sem=rsem.at[slot],
                device_id=(dst,), device_id_type=MESH)

        def head_copy():
            return pltpu.make_async_remote_copy(
                src_ref=sbuf.at[pl.ds(0, _HEAD_ROWS)], dst_ref=hbuf.at[pl.ds(0, _HEAD_ROWS)],
                send_sem=ssem.at[4], recv_sem=rsem.at[3], device_id=(0,), device_id_type=MESH)

        def thr_copy():
            return pltpu.make_async_remote_copy(
                src_ref=tbuf, dst_ref=tbuf, send_sem=ssem.at[4], recv_sem=rsem.at[3],
                device_id=(2,), device_id_type=MESH)

        @pl.when(me % 2 == 0)
        def _():
            cin.wait()

        g = _rotate_regs([xin[pl.ds(8 * k, 8), :] for k in range(8)], lbit)
        g = [_perm(g[k], idx_in[k]) for k in range(8)]
        v = (_insertion_sort([_skew(g[k], k) for k in range(8)])
             + _insertion_sort([_skew(g[k], 64 + k) for k in range(8)]))
        for i, j in _MERGE_8_8:
            _ce(v, i, j)
        v = [(v[i], tuple(i | (s >> 2) << 4 | ((s >> 1) & 1) << 5 | (s & 1) << 6 for s in range(8)))
             for i in range(16)]
        v = net.stage(v, 31, 4, first=1)
        for mu in (8, 4, 2):
            v = net.stage(v, mu)
        v = net.swap_stage(v, 1, 4, 2)
        v = net.stage(v, 63, 6, first=1)
        for mu in (16, 8, 4):
            v = net.stage(v, mu)
        v = net.swap_stage(v, 2, 4, 4)
        v = net.swap_stage(v, 1, 2, 2)
        top = net.align(v, 127, 7, 1)

        def finish(h, half):
            for mu in (32, 16, 8):
                h = net.stage(h, mu)
            h = net.swap_stage(h, 4, 4, 8)
            h = net.swap_stage(h, 2, 2, 4)
            y = {}
            for a, b in net.swap(h, 1, 2):
                lo, hi = net.lo(a, b, 1), net.hi(a, b, 1)
                assert lo[1] == tuple(lo[1][0] | s << 1 for s in range(8))
                y[lo[1][0] & 63] = jnp.where(hlo, lo[0], hi[0])
            for k in range(4):
                sbuf[pl.ds(16 * half + 4 * k, 4), :] = pltpu.bitcast(y[16 * k].astype(BF16), U32)

        finish([net.lo(a, b, 127) for a, b in top], 0)

        @pl.when(me == 2)
        def _():
            head_copy().start()

        finish([net.hi(a, b, 127) for a, b in top], 1)

        @pl.when(me == 2)
        def _():
            rcopy(2, 3).start()
            rcopy(2, 1).start()

        @pl.when(me == 0)
        def _():
            pl.semaphore_wait(rdy, 2)
            rcopy(0, 1).start()
            rcopy(0, 3).start()
            pl.semaphore_wait(bar, 1)
            rcopy(0, 2).start()

        @pl.when(me == 1)
        def _():
            rcopy(1, 0).start()
            pl.semaphore_wait(rdy, 1)
            rcopy(1, 3).start()
            rcopy(1, 2).start()

        @pl.when(me == 3)
        def _():
            rcopy(3, 0).start()
            pl.semaphore_wait(rdy, 1)
            rcopy(3, 1).start()
            rcopy(3, 2).start()

        def unpack(ref, xor, n=4):
            out = []
            for k in range(n):
                w = ref[pl.ds(8 * k, 8), :]
                if xor is not None:
                    w = w ^ xor
                f = pltpu.bitcast(w, BF16).astype(F32)
                out += [f[:8], f[8:]]
            return out

        def merge7(v, desc=False):
            v = list(v)
            for d in (4, 2, 1):
                _vstage(v, d, desc)
            out, big = [], []
            for a in v:
                for d in (4, 2, 1):
                    a = _pick(net.low[d], a, net.xor_val(a, d), desc)
                r = pltpu.roll(a, 64, 1)
                out.append(_pick(hlo, a, r, desc))
                big.append(jnp.maximum(a, r))
            return out, big

        neg = jnp.uint32(0x80008000)
        own = unpack(sbuf, None)
        rcopy(1, 0).wait_recv()
        a = unpack(rbuf.at[0], neg)
        m0, _ = merge7([jnp.minimum(p, q) for p, q in zip(own, a)])
        m1, _ = merge7([jnp.maximum(p, q) for p, q in zip(own, a)])
        rcopy(3, 0).wait_recv()
        b = unpack(rbuf.at[1], neg)
        edge = jnp.logical_or(me == 0, me == 3)
        pp = [jnp.where(edge, jnp.minimum(p, q), jnp.maximum(p, q)) for p, q in zip(m0, b)]
        qq = [jnp.where(edge, -jnp.inf, p) for p in m1]
        u, ubig = merge7([jnp.maximum(p, q) for p, q in zip(pp, qq)], desc=True)
        l, _ = merge7([jnp.minimum(p, q) for p, q in zip(pp, qq)], desc=True)

        last = 4 * _HEAD_ROWS - 1
        assert last >> 4 == (last + 1) >> 4 == 3
        row = (last >> 1) & 7

        def need_rest(d3, thr):
            ok = jnp.logical_or(hlo[:1], d3[row:row + 1] >= thr)
            return jnp.max(jnp.where(ok, 0.0, 1.0)) > 0.0

        z = [4 * sub + k + (lane >> 1) for k in range(5)]
        idx_pre = [(t >> 2) & 7 for t in z]
        m_pre = [(t & 32) != 0 for t in z]

        def emit(v, rolled=0):
            idx_out = [(((lane - j) >> 3) - sub) & 7 for j in range(8)]
            for j in range(8 - rolled, 8):
                idx_out[j] = pltpu.roll(idx_out[0], j, 1)
            h = [(v[i], tuple(i << 4 | s << 1 for s in range(8))) for i in range(8)]
            for mu in (32, 16):
                h = net.stage(h, mu)
            h = net.swap_stage(h, 8, 4, 32)
            h = net.swap_stage(h, 4, 2, 16)
            h = net.swap_stage(h, 2, 1, 8)
            f = [[None] * 4 for _ in range(2)]
            for val, pos in h:
                assert pos == tuple(pos[0] | s << 3 for s in range(8))
                f[pos[0] >> 6][(pos[0] >> 1) & 3] = val
            f = [_rotate_regs(r, lbit[1:]) for r in f]
            f = [[_perm(r[k % 4], idx_pre[k]) for k in range(5)] for r in f]
            g0 = [[jnp.where(m_pre[k], f[1 - c][k], f[c][k]) for k in range(5)] for c in range(2)]
            r = []
            for j in range(8):
                k = j // 2
                t = [_skew(jnp.where(lbit[0], g0[c][k + 1], g0[c][k]) if j % 2 else g0[c][k], 64 * c + j)
                     for c in range(2)]
                rr = jnp.where(lbit[0], jnp.maximum(t[0], t[1]), jnp.minimum(t[0], t[1]))
                r.append(_perm(rr, idx_out[j]))
            o = _rotate_regs([r[(-k) % 8] for k in range(8)], lbit, sign=-1)
            for k in range(8):
                obuf[pl.ds(8 * k, 8), :] = o[k]

        def full(lo, hi, dxor):
            rcopy(2, 0).wait_recv()
            d = unpack(rbuf.at[2], dxor)
            f = [jnp.minimum(h, p) for p, h in zip(d, hi)]
            if lo is not None:
                f = [jnp.maximum(p, q) for p, q in zip(f, lo)]
            _vstage(f, 4)
            emit(f)

        @pl.when(me != 0)
        def _():
            sgn = (1 - 2 * (me % 2)).astype(F32)
            us = [p * sgn for p in u]
            ls = [p * sgn for p in l]
            full([jnp.minimum(p, q) for p, q in zip(us, ls)],
                 [jnp.maximum(p, q) for p, q in zip(us, ls)],
                 (me % 2).astype(U32) * neg)

            @pl.when(me == 2)
            def _():
                head_copy().wait_send()
                rcopy(2, 1).wait_send()
                rcopy(2, 3).wait_send()
                thr_copy().wait_recv()

                @pl.when(need_rest(own[3], tbuf[...]))
                def _():
                    rcopy(2, 0).start()
                    rcopy(2, 0).wait_send()

            @pl.when(me == 1)
            def _():
                for dst in (0, 2, 3):
                    rcopy(1, dst).wait_send()

            @pl.when(me == 3)
            def _():
                for dst in (0, 1, 2):
                    rcopy(3, dst).wait_send()

        @pl.when(me == 0)
        def _():
            thr = ubig[3][row + 1:row + 2]
            tbuf[...] = thr
            thr_copy().start()
            for dst in (1, 2, 3):
                rcopy(0, dst).wait_send()
            thr_copy().wait_send()
            head_copy().wait_recv()
            d = unpack(hbuf, None, n=2)
            more = need_rest(d[3], thr)
            f = [jnp.minimum(d[i], u[4 + i]) for i in range(4)]
            f += [jnp.maximum(jnp.minimum(d[i], u[i]), u[4 + i]) for i in range(4)]
            emit(f, rolled=3)

            @pl.when(more)
            def _():
                full(None, u, None)

    out = pl.pallas_call(
        body,
        out_shape=jax.ShapeDtypeStruct((64, 128), F32),
        in_specs=[pl.BlockSpec(memory_space=pl.ANY)],
        out_specs=pl.BlockSpec(memory_space=pltpu.VMEM),
        scratch_shapes=[
            pltpu.VMEM((64, 128), F32),
            pltpu.VMEM((32, 128), U32),
            pltpu.VMEM((3, 32, 128), U32),
            pltpu.VMEM((16, 128), U32),
            pltpu.VMEM((1, 128), F32),
            pltpu.SemaphoreType.DMA,
            pltpu.SemaphoreType.DMA((5,)),
            pltpu.SemaphoreType.DMA((4,)),
            pltpu.SemaphoreType.REGULAR,
        ],
        compiler_params=pltpu.CompilerParams(collective_id=0, disable_semaphore_checks=True),
    )(x.T)
    return out.T
```

```python
import jax
import jax.numpy as jnp
from jax import lax
from jax.experimental import pallas as pl
from jax.experimental.pallas import tpu as pltpu

MESH = pl.DeviceIdType.MESH
F32 = jnp.float32
BF16 = jnp.bfloat16
U32 = jnp.uint32

_SLOT = {
    0: {1: 0, 3: 1, 2: 2},
    1: {0: 0, 2: 1, 3: 2},
    3: {0: 0, 2: 1, 1: 2},
    2: {1: 0, 3: 1, 0: 2},
}


def _odd_even_merge(lo, n, r):
    m = 2 * r
    if m < n:
        yield from _odd_even_merge(lo, n, m)
        yield from _odd_even_merge(lo + r, n, m)
        for i in range(lo + r, lo + n - r, m):
            yield (i, i + r)
    else:
        yield (lo, lo + r)


_MERGE_8_8 = sorted(_odd_even_merge(0, 16, 1), key=lambda p: p[0] - p[1])


def _insertion_sort(xs):
    out = [xs[0]]
    for x in xs[1:]:
        mins = [jnp.minimum(p, x) for p in out] + [x]
        out = [mins[0]] + [jnp.maximum(p, q) for p, q in zip(out, mins[1:])]
    return out


def _perm(x, idx):
    return jnp.take_along_axis(x, idx, axis=0, mode="promise_in_bounds")


class _Net:
    def __init__(self, sub):
        self.low = {d: (sub & d) == 0 for d in (4, 2, 1)}
        self.idx = {d: sub ^ d for d in (1, 2, 6, 7)}

    def xor_val(self, x, d):
        return pltpu.roll(x, 4, 0) if d == 4 else _perm(x, self.idx[d])

    def xor(self, a, d):
        return self.xor_val(a[0], d), tuple(a[1][s ^ d] for s in range(8))

    def sel(self, d, a, b):
        return (jnp.where(self.low[d], a[0], b[0]),
                tuple(b[1][s] if s & d else a[1][s] for s in range(8)))

    @staticmethod
    def lo(a, b, mu):
        assert all(p ^ q == mu for p, q in zip(a[1], b[1]))
        return jnp.minimum(a[0], b[0]), tuple(min(p, q) for p, q in zip(a[1], b[1]))

    @staticmethod
    def hi(a, b, mu):
        assert all(p ^ q == mu for p, q in zip(a[1], b[1]))
        return jnp.maximum(a[0], b[0]), tuple(max(p, q) for p, q in zip(a[1], b[1]))

    @staticmethod
    def pairs(v, mu, d=0, first=0):
        out, used = [], set()
        for i in sorted(range(len(v)), key=lambda i: bool(v[i][1][0] & first)):
            if i in used:
                continue
            want = tuple(v[i][1][s ^ d] ^ mu for s in range(8))
            j = next(j for j in range(len(v)) if v[j][1] == want)
            assert j != i and j not in used
            used.update((i, j))
            out.append((v[i], v[j]))
        return out

    def align(self, v, mu, d, first):
        return [(a, self.xor(b, d) if d else b) for a, b in self.pairs(v, mu, d, first)]

    def both(self, pairs, mu):
        out = []
        for a, b in pairs:
            out += [self.lo(a, b, mu), self.hi(a, b, mu)]
        return out

    def stage(self, v, mu, d=0, first=0):
        return self.both(self.align(v, mu, d, first), mu)

    def swap(self, v, d, nu):
        return [(self.sel(d, a, b), self.xor(self.sel(d, b, a), d))
                for a, b in self.pairs(v, nu, first=nu)]

    def swap_stage(self, v, mu, d, nu):
        return self.both(self.swap(v, d, nu), mu)


def _ce(v, i, j, desc=False):
    lo = jnp.minimum(v[i], v[j])
    hi = jnp.maximum(v[i], v[j])
    v[i], v[j] = (hi, lo) if desc else (lo, hi)


def _vstage(v, d, desc=False):
    for i in range(len(v)):
        if not i & d:
            _ce(v, i, i | d, desc)


def _pick(low, x, p, desc=False):
    if desc:
        return jnp.where(low, jnp.maximum(x, p), jnp.minimum(x, p))
    return jnp.where(low, jnp.minimum(x, p), jnp.maximum(x, p))


def _rotate_regs(v, masks, sign=1):
    n = len(v)
    for b, m in enumerate(masks):
        v = [jnp.where(m, v[(k + sign * (1 << b)) % n], v[k]) for k in range(n)]
    return v


def _skew(x, base):
    return pltpu.roll(x, base, 1, stride=8, stride_axis=0)


def pallas_dist_sort_i_m128_n64_kernel(x: jax.Array):
    def body(x_hbm, obuf, xin, sbuf, rbuf, hbuf, tbuf, lsem, ssem, rsem, rdy):
        me = lax.axis_index("i")
        cin = pltpu.make_async_copy(x_hbm, xin, lsem)
        cin.start()

        bar = pltpu.get_barrier_semaphore()

        def sig(sem, dst):
            pl.semaphore_signal(sem, inc=1, device_id=(dst,), device_id_type=MESH)

        @pl.when(me == 0)
        def _():
            sig(bar, 2)
            sig(bar, 1)
            sig(bar, 3)

        @pl.when(me == 2)
        def _():
            sig(bar, 0)
            pl.semaphore_wait(bar, 3)
            sig(rdy, 1)
            sig(rdy, 3)

        @pl.when(me % 2 == 1)
        def _():
            sig(bar, 2)
            pl.semaphore_wait(bar, 1)
            sig(rdy, 0)
            cin.wait()
            xin[...] = -xin[...]

        sub = lax.broadcasted_iota(jnp.int32, (8, 128), 0)
        lane = lax.broadcasted_iota(jnp.int32, (8, 128), 1)
        net = _Net(sub)
        hlo = lane < 64
        lbit = [(lane & (1 << b)) != 0 for b in range(3)]
        idx_in = [(((lane + k) >> 3) + sub) & 7 for k in range(8)]

        def rcopy(src, dst):
            slot = _SLOT[dst][src]
            return pltpu.make_async_remote_copy(
                src_ref=sbuf, dst_ref=rbuf.at[slot], send_sem=ssem.at[dst], recv_sem=rsem.at[slot],
                device_id=(dst,), device_id_type=MESH)

        def head_copy(k):
            rows = pl.ds(*((0, 4), (4, 8), (12, 4))[k])
            return pltpu.make_async_remote_copy(
                src_ref=sbuf.at[rows], dst_ref=hbuf.at[rows],
                send_sem=ssem.at[4 + k], recv_sem=rsem.at[3 + k],
                device_id=(0,), device_id_type=MESH)

        def thr_copy():
            return pltpu.make_async_remote_copy(
                src_ref=tbuf, dst_ref=tbuf, send_sem=ssem.at[4], recv_sem=rsem.at[3],
                device_id=(2,), device_id_type=MESH)

        @pl.when(me % 2 == 0)
        def _():
            cin.wait()

        g = _rotate_regs([xin[pl.ds(8 * k, 8), :] for k in range(8)], lbit)
        g = [_perm(g[k], idx_in[k]) for k in range(8)]
        v = (_insertion_sort([_skew(g[k], k) for k in range(8)])
             + _insertion_sort([_skew(g[k], 64 + k) for k in range(8)]))
        for i, j in _MERGE_8_8:
            _ce(v, i, j)
        v = [(v[i], tuple(i | (s >> 2) << 4 | ((s >> 1) & 1) << 5 | (s & 1) << 6 for s in range(8)))
             for i in range(16)]
        pairs32 = net.align(v, 31, 4, 1)

        def run32(h):
            for mu in (8, 4, 2):
                h = net.stage(h, mu)
            return net.swap_stage(h, 1, 4, 2)

        v = run32([net.lo(a, b, 31) for a, b in pairs32])

        def put(a, b):
            lo, hi = net.lo(a, b, 1), net.hi(a, b, 1)
            assert lo[1] == tuple(lo[1][0] | s << 1 for s in range(8))
            y = jnp.where(hlo, lo[0], hi[0])
            sbuf[pl.ds(lo[1][0] // 4, 4), :] = pltpu.bitcast(y.astype(BF16), U32)

        h = [net.lo(a, b, 47) for a, b in net.align(v, 47, 6, 1)]
        for mu in (8, 4):
            h = net.stage(h, mu)
        h = net.swap_stage(h, 2, 4, 4)
        h = net.swap_stage(h, 1, 2, 2)
        h = [net.lo(a, b, 79) for a, b in net.align(h, 79, 7, 1)]
        h = net.stage(h, 8)
        h = net.swap_stage(h, 4, 4, 8)
        h = net.swap_stage(h, 2, 2, 4)
        put(*net.swap(h, 1, 2)[0])

        @pl.when(me == 2)
        def _():
            head_copy(0).start()

        v = v + run32([net.hi(a, b, 31) for a, b in pairs32])
        v = net.stage(v, 63, 6, first=1)
        for mu in (16, 8, 4):
            v = net.stage(v, mu)
        v = net.swap_stage(v, 2, 4, 4)
        v = net.swap_stage(v, 1, 2, 2)
        top = net.align(v, 127, 7, 1)

        def finish(h):
            for mu in (32, 16, 8):
                h = net.stage(h, mu)
            h = net.swap_stage(h, 4, 4, 8)
            h = net.swap_stage(h, 2, 2, 4)
            for a, b in net.swap(h, 1, 2):
                if a[1][0] >= 16:
                    put(a, b)

        finish([net.lo(a, b, 127) for a, b in top])

        @pl.when(me == 2)
        def _():
            head_copy(1).start()
            head_copy(2).start()

        finish([net.hi(a, b, 127) for a, b in top])

        @pl.when(me == 2)
        def _():
            rcopy(2, 3).start()
            rcopy(2, 1).start()

        @pl.when(me == 0)
        def _():
            pl.semaphore_wait(rdy, 2)
            rcopy(0, 1).start()
            rcopy(0, 3).start()
            pl.semaphore_wait(bar, 1)
            rcopy(0, 2).start()

        @pl.when(me == 1)
        def _():
            rcopy(1, 0).start()
            pl.semaphore_wait(rdy, 1)
            rcopy(1, 3).start()
            rcopy(1, 2).start()

        @pl.when(me == 3)
        def _():
            rcopy(3, 0).start()
            pl.semaphore_wait(rdy, 1)
            rcopy(3, 1).start()
            rcopy(3, 2).start()

        def unpack(ref, xor, n=4):
            out = []
            for k in range(n):
                w = ref[pl.ds(8 * k, 8), :]
                if xor is not None:
                    w = w ^ xor
                f = pltpu.bitcast(w, BF16).astype(F32)
                out += [f[:8], f[8:]]
            return out

        def merge7(v, desc=False):
            v = list(v)
            for d in (4, 2, 1):
                _vstage(v, d, desc)
            out, big = [], []
            for a in v:
                for d in (4, 2, 1):
                    a = _pick(net.low[d], a, net.xor_val(a, d), desc)
                r = pltpu.roll(a, 64, 1)
                out.append(_pick(hlo, a, r, desc))
                big.append(jnp.maximum(a, r))
            return out, big

        neg = jnp.uint32(0x80008000)
        own = unpack(sbuf, None)
        rcopy(1, 0).wait_recv()
        a = unpack(rbuf.at[0], neg)
        m0, _ = merge7([jnp.minimum(p, q) for p, q in zip(own, a)])
        m1, _ = merge7([jnp.maximum(p, q) for p, q in zip(own, a)])
        rcopy(3, 0).wait_recv()
        b = unpack(rbuf.at[1], neg)
        edge = jnp.logical_or(me == 0, me == 3)
        pp = [jnp.where(edge, jnp.minimum(p, q), jnp.maximum(p, q)) for p, q in zip(m0, b)]
        qq = [jnp.where(edge, -jnp.inf, p) for p in m1]
        u, ubig = merge7([jnp.maximum(p, q) for p, q in zip(pp, qq)], desc=True)
        l, _ = merge7([jnp.minimum(p, q) for p, q in zip(pp, qq)], desc=True)

        def need_more(dreg, thr):
            ok = jnp.logical_or(hlo[:1], dreg[7:] >= thr)
            return jnp.max(jnp.where(ok, 0.0, 1.0)) > 0.0

        z = [4 * sub + k + (lane >> 1) for k in range(5)]
        idx_pre = [(t >> 2) & 7 for t in z]
        m_pre = [(t & 32) != 0 for t in z]

        def emit(v, rolled=0):
            idx_out = [(((lane - j) >> 3) - sub) & 7 for j in range(8)]
            for j in range(8 - rolled, 8):
                idx_out[j] = pltpu.roll(idx_out[0], j, 1)
            h = [(v[i], tuple(i << 4 | s << 1 for s in range(8))) for i in range(8)]
            for mu in (32, 16):
                h = net.stage(h, mu)
            h = net.swap_stage(h, 8, 4, 32)
            h = net.swap_stage(h, 4, 2, 16)
            h = net.swap_stage(h, 2, 1, 8)
            f = [[None] * 4 for _ in range(2)]
            for val, pos in h:
                assert pos == tuple(pos[0] | s << 3 for s in range(8))
                f[pos[0] >> 6][(pos[0] >> 1) & 3] = val
            f = [_rotate_regs(r, lbit[1:]) for r in f]
            f = [[_perm(r[k % 4], idx_pre[k]) for k in range(5)] for r in f]
            g0 = [[jnp.where(m_pre[k], f[1 - c][k], f[c][k]) for k in range(5)] for c in range(2)]
            r = []
            for j in range(8):
                k = j // 2
                t = [_skew(jnp.where(lbit[0], g0[c][k + 1], g0[c][k]) if j % 2 else g0[c][k], 64 * c + j)
                     for c in range(2)]
                rr = jnp.where(lbit[0], jnp.maximum(t[0], t[1]), jnp.minimum(t[0], t[1]))
                r.append(_perm(rr, idx_out[j]))
            o = _rotate_regs([r[(-k) % 8] for k in range(8)], lbit, sign=-1)
            for k in range(8):
                obuf[pl.ds(8 * k, 8), :] = o[k]

        def full(lo, hi, dxor):
            rcopy(2, 0).wait_recv()
            d = unpack(rbuf.at[2], dxor)
            f = [jnp.minimum(h, p) for p, h in zip(d, hi)]
            if lo is not None:
                f = [jnp.maximum(p, q) for p, q in zip(f, lo)]
            _vstage(f, 4)
            emit(f)

        @pl.when(me != 0)
        def _():
            sgn = (1 - 2 * (me % 2)).astype(F32)
            us = [p * sgn for p in u]
            ls = [p * sgn for p in l]
            full([jnp.minimum(p, q) for p, q in zip(us, ls)],
                 [jnp.maximum(p, q) for p, q in zip(us, ls)],
                 (me % 2).astype(U32) * neg)

            @pl.when(me == 2)
            def _():
                for k in range(3):
                    head_copy(k).wait_send()
                rcopy(2, 1).wait_send()
                rcopy(2, 3).wait_send()
                thr_copy().wait_recv()

                @pl.when(jnp.logical_and(need_more(own[2], tbuf[pl.ds(0, 1), :]),
                                         need_more(own[3], tbuf[pl.ds(1, 1), :])))
                def _():
                    rcopy(2, 0).start()
                    rcopy(2, 0).wait_send()

            @pl.when(me == 1)
            def _():
                for dst in (0, 2, 3):
                    rcopy(1, dst).wait_send()

            @pl.when(me == 3)
            def _():
                for dst in (0, 1, 2):
                    rcopy(3, dst).wait_send()

        @pl.when(me == 0)
        def _():
            tbuf[pl.ds(0, 1), :] = ubig[3][:1]
            tbuf[pl.ds(1, 1), :] = ubig[4][:1]
            thr_copy().start()
            for dst in (1, 2, 3):
                rcopy(0, dst).wait_send()
            thr_copy().wait_send()

            def with_head(n, rolled):
                d = [pltpu.bitcast(hbuf[pl.ds(4 * k, 4), :], BF16).astype(F32) for k in range(n)]
                more = need_more(d[n - 1], ubig[n][:1])
                f = [jnp.minimum(p, q) for p, q in zip(d, u[4:])] + u[4 + n:]
                f += [jnp.maximum(jnp.minimum(p, q), r) for p, q, r in zip(d, u, u[4:])] + u[n:4]
                emit(f, rolled)
                return more

            head_copy(0).wait_recv()
            head_copy(1).wait_recv()
            more = with_head(3, 3)

            @pl.when(more)
            def _():
                head_copy(2).wait_recv()

                @pl.when(with_head(4, 0))
                def _():
                    full(None, u, None)

            @pl.when(jnp.logical_not(more))
            def _():
                head_copy(2).wait_recv()

    out = pl.pallas_call(
        body,
        out_shape=jax.ShapeDtypeStruct((64, 128), F32),
        in_specs=[pl.BlockSpec(memory_space=pl.ANY)],
        out_specs=pl.BlockSpec(memory_space=pltpu.VMEM),
        scratch_shapes=[
            pltpu.VMEM((64, 128), F32),
            pltpu.VMEM((32, 128), U32),
            pltpu.VMEM((3, 32, 128), U32),
            pltpu.VMEM((16, 128), U32),
            pltpu.VMEM((2, 128), F32),
            pltpu.SemaphoreType.DMA,
            pltpu.SemaphoreType.DMA((7,)),
            pltpu.SemaphoreType.DMA((6,)),
            pltpu.SemaphoreType.REGULAR,
        ],
        compiler_params=pltpu.CompilerParams(collective_id=0, disable_semaphore_checks=True),
    )(x.T)
    return out.T
```
